```python
import numpy as np

kernel_name = "dist_ag_xy_y_m1024_n512"

def setup_inputs():
    return {"x": np.random.randn(2048, 512).astype(np.float32)}

def reference(x: np.ndarray) -> np.ndarray:
    return x
```

```python
import functools
import jax
import jax.numpy as jnp
from jax import lax
from jax.experimental import pallas as pl
from jax.experimental.pallas import tpu as pltpu

MESH = pl.DeviceIdType.MESH

def make(C=16, F=464, margin=4, groups=(1, 2, 4, 8), K=8, per=2):
    def kernel(x):
        m, n = x.shape
        S = m - F
        nF = F // C
        nMid = (S - F) // C
        nS = nF + nMid
        assert F % C == 0 and (S - F) % C == 0
        gl = []
        j = 0; gi = 0
        while j < nF:
            g = min(groups[min(gi, len(groups) - 1)], nF - j)
            gl.append((j, g)); j += g; gi += 1
        if nMid: gl.append((nF, nMid))
        nG = len(gl)
        first_of_group = {j0: gi for gi, (j0, g) in enumerate(gl)}
        def body(x_ref, out_ref, sbuf, rbuf, lsem, ssem, rsem, fssem, frsem, xready):
            mx = lax.axis_index("x"); my = lax.axis_index("y")
            ynbr = (mx, 1 - my); xnbr = (1 - mx, my)
            bar = pltpu.get_barrier_semaphore()
            own = my * m
            oth = (1 - my) * m
            sbase = mx * S
            fbase = (1 - mx) * S
            def soff(j):
                if j < nF:
                    return pl.multiple_of(sbase + j * C, C)
                return F + (j - nF) * C
            def foff(j):
                return pl.multiple_of(fbase + j * C, C)
            loads = []
            for gi, (j0, g) in enumerate(gl):
                loads.append(pltpu.make_async_copy(x_ref.at[pl.ds(soff(j0), g * C)], out_ref.at[pl.ds(pl.multiple_of(own + soff(j0), C), g * C)], lsem.at[gi]))
            rest = pltpu.make_async_copy(x_ref.at[pl.ds(foff(0), F)], out_ref.at[pl.ds(pl.multiple_of(own + foff(0), C), F)], lsem.at[nG])
            loads[0].start()
            pl.semaphore_signal(bar, inc=1, device_id=ynbr, device_id_type=MESH)
            @pl.when(mx == 0)
            def _():
                pl.semaphore_signal(bar, inc=1, device_id=xnbr, device_id_type=MESH)
            for gi in range(1, nG):
                loads[gi].start()
            rest.start()
            def ydesc(j):
                return pltpu.make_async_remote_copy(src_ref=sbuf.at[pl.ds(soff(j), C)], dst_ref=rbuf.at[pl.ds(soff(j), C)],
                          send_sem=ssem, recv_sem=rsem.at[j], device_id=ynbr, device_id_type=MESH)
            def send(j):
                if j in first_of_group:
                    loads[first_of_group[j]].wait()
                sbuf[pl.ds(soff(j), C), :] = out_ref[pl.ds(pl.multiple_of(own + soff(j), C), C), :].astype(jnp.bfloat16)
                if j == 0:
                    pl.semaphore_wait(bar, 1 + mx)
                ydesc(j).start()
                if j == 0:
                    @pl.when(mx == 1)
                    def _():
                        pl.semaphore_signal(xready, inc=1, device_id=xnbr, device_id_type=MESH)
            def xproc(j):
                f = pltpu.make_async_remote_copy(src_ref=rbuf.at[pl.ds(foff(j), C)], dst_ref=rbuf.at[pl.ds(foff(j), C)],
                          send_sem=fssem, recv_sem=frsem.at[j], device_id=xnbr, device_id_type=MESH)
                f.wait_recv()
                out_ref[pl.ds(pl.multiple_of(oth + foff(j), C), C), :] = rbuf[pl.ds(foff(j), C), :].astype(jnp.float32)
            sent = 0
            while sent < min(K, nS):
                send(sent); sent += 1
            xdone = 0
            for j in range(nS):
                if j == nS - 1:
                    pltpu.make_async_copy(sbuf.at[pl.ds(0, S)], sbuf.at[pl.ds(0, S)], ssem).wait()
                    rest.wait()
                ydesc(j).wait_recv()
                if j < nF:
                    if j == 0:
                        @pl.when(mx == 0)
                        def _():
                            pl.semaphore_wait(xready, 1)
                    pltpu.make_async_remote_copy(src_ref=rbuf.at[pl.ds(soff(j), C)], dst_ref=rbuf.at[pl.ds(soff(j), C)],
                          send_sem=fssem, recv_sem=frsem.at[j], device_id=xnbr, device_id_type=MESH).start()
                for _ in range(per):
                    if sent < nS:
                        send(sent); sent += 1
                out_ref[pl.ds(pl.multiple_of(oth + soff(j), C), C), :] = rbuf[pl.ds(soff(j), C), :].astype(jnp.float32)
                lag = nMid + (margin if j < nF - 1 else 0)
                while xdone <= j - lag and xdone < nF - 1:
                    xproc(xdone); xdone += 1
            while xdone < nF - 1:
                xproc(xdone); xdone += 1
            pltpu.make_async_copy(rbuf.at[pl.ds(0, F)], rbuf.at[pl.ds(0, F)], fssem).wait()
            xproc(nF - 1)
        return pl.pallas_call(
            body,
            out_shape=jax.ShapeDtypeStruct((2 * m, n), x.dtype),
            in_specs=[pl.BlockSpec(memory_space=pl.ANY)],
            out_specs=pl.BlockSpec(memory_space=pltpu.VMEM),
            scratch_shapes=[pltpu.VMEM((m, n), jnp.bfloat16), pltpu.VMEM((m, n), jnp.bfloat16),
                            pltpu.SemaphoreType.DMA((nG + 1,)), pltpu.SemaphoreType.DMA, pltpu.SemaphoreType.DMA((nS,)),
                            pltpu.SemaphoreType.DMA, pltpu.SemaphoreType.DMA((nF,)), pltpu.SemaphoreType.REGULAR],
            compiler_params=pltpu.CompilerParams(collective_id=0, disable_semaphore_checks=True, disable_bounds_checks=True),
        )(x)
    return kernel


_KERNEL = make(F=464, K=6)


def pallas_dist_ag_xy_y_m1024_n512_kernel(x: jax.Array):
    return _KERNEL(x)
```

```python
import jax
import jax.numpy as jnp
from jax import lax
from jax.experimental import pallas as pl
from jax.experimental.pallas import tpu as pltpu

_MESH = pl.DeviceIdType.MESH

_C = 16
_W = 128
_N_FWD = 29
_W_FWD = 256
_LOAD_GROUPS = (1, 2, 4, 8)
_N_PRIME = 8
_SENDS_PER_STEP = 2
_X_MARGIN = 6


def _compiler_params():
    try:
        return pltpu.CompilerParams(
            collective_id=0,
            disable_semaphore_checks=True,
            disable_bounds_checks=True,
        )
    except TypeError:
        return pltpu.CompilerParams(collective_id=0)


def pallas_dist_ag_xy_y_m1024_n512_kernel(
x: jax.Array,
):
    m, n = x.shape
    C, W, nF, Wf = _C, _W, _N_FWD, _W_FWD
    NC = n // W
    F = nF * C
    S = m - F
    nMid = (S - F) // C
    nS = nF + nMid
    nBp = Wf // W
    nBd = 1 if n - 2 * Wf > 0 else 0
    assert m % C == 0 and n % W == 0 and nMid >= 2 and 0 < 2 * Wf <= n

    groups = []
    j = 0
    while j < nF:
        g = min(_LOAD_GROUPS[min(len(groups), len(_LOAD_GROUPS) - 1)], nF - j)
        groups.append((j, g))
        j += g
    groups.append((nF, nMid))
    nG = len(groups)
    assert groups[0][1] == 1
    group_of_first_chunk = {j0: gi for gi, (j0, _) in enumerate(groups)}

    def body(x_ref, out_ref, sbuf, rbuf, lsem, ssem, bssem, rsem, fssem, bfssem,
             frsem, xready):
        mx = lax.axis_index("x")
        my = lax.axis_index("y")
        ynbr = (mx, 1 - my)
        xnbr = (1 - mx, my)
        bar = pltpu.get_barrier_semaphore()
        own = my * m
        oth = (1 - my) * m
        sbase = mx * S
        fbase = (1 - mx) * S

        def soff(j):
            if j < nF:
                return pl.multiple_of(sbase + j * C, C)
            return F + (j - nF) * C

        def foff(j):
            return pl.multiple_of(fbase + j * C, C)

        def rows(base, off, size):
            return pl.ds(pl.multiple_of(base + off, C), size)

        load00 = pltpu.make_async_copy(
            x_ref.at[pl.ds(soff(0), C), pl.ds(0, W)],
            out_ref.at[rows(own, soff(0), C), pl.ds(0, W)],
            lsem.at[nG + 1])
        loads = [pltpu.make_async_copy(
            x_ref.at[pl.ds(soff(0), C), pl.ds(W, n - W)],
            out_ref.at[rows(own, soff(0), C), pl.ds(W, n - W)],
            lsem.at[0])]
        for gi in range(1, nG):
            j0, g = groups[gi]
            loads.append(pltpu.make_async_copy(
                x_ref.at[pl.ds(soff(j0), g * C)],
                out_ref.at[rows(own, soff(j0), g * C)],
                lsem.at[gi]))
        rest = pltpu.make_async_copy(
            x_ref.at[pl.ds(foff(0), F)],
            out_ref.at[rows(own, foff(0), F)],
            lsem.at[nG])

        load00.start()
        pl.semaphore_signal(bar, inc=1, device_id=ynbr, device_id_type=_MESH)

        @pl.when(mx == 0)
        def _():
            pl.semaphore_signal(bar, inc=1, device_id=xnbr, device_id_type=_MESH)

        for cp in loads:
            cp.start()
        rest.start()

        items = {}
        ri = 0
        fi = 0
        for j in range(nS):
            lst = []
            if j < nF:
                for p in range(NC):
                    lst.append((p * W, W, True, ri, fi, ssem, fssem))
                    ri += 1
                    fi += 1
            elif j == nF:
                for p in range(nBp):
                    c0 = pl.multiple_of(mx * (n - Wf) + p * W, W)
                    lst.append((c0, W, True, ri, fi, bssem.at[p], bfssem.at[p]))
                    ri += 1
                    fi += 1
                if nBd:
                    lst.append((Wf, n - 2 * Wf, False, ri, None, bssem.at[nBp], None))
                    ri += 1
            else:
                lst.append((0, n, False, ri, None, ssem, None))
                ri += 1
            items[j] = lst

        def ydesc(j, it):
            c0, w, _, r, _, ss, _ = it
            return pltpu.make_async_remote_copy(
                src_ref=sbuf.at[pl.ds(soff(j), C), pl.ds(c0, w)],
                dst_ref=rbuf.at[pl.ds(soff(j), C), pl.ds(c0, w)],
                send_sem=ss, recv_sem=rsem.at[r],
                device_id=ynbr, device_id_type=_MESH)

        def fdesc(j, it):
            c0, w, _, _, f, _, fs = it
            return pltpu.make_async_remote_copy(
                src_ref=rbuf.at[pl.ds(soff(j), C), pl.ds(c0, w)],
                dst_ref=rbuf.at[pl.ds(soff(j), C), pl.ds(c0, w)],
                send_sem=fs, recv_sem=frsem.at[f],
                device_id=xnbr, device_id_type=_MESH)

        def send(j):
            if j == 0:
                load00.wait()
                sbuf[pl.ds(soff(0), C), pl.ds(0, W)] = out_ref[
                    rows(own, soff(0), C), pl.ds(0, W)].astype(jnp.bfloat16)

                @pl.when(mx == 0)
                def _():
                    pl.semaphore_wait(bar, 1)

                @pl.when(mx == 1)
                def _():
                    pl.semaphore_wait(bar, 2)

                ydesc(0, items[0][0]).start()
                loads[0].wait()
                sbuf[pl.ds(soff(0), C), pl.ds(W, n - W)] = out_ref[
                    rows(own, soff(0), C), pl.ds(W, n - W)].astype(jnp.bfloat16)
                for it in items[0][1:]:
                    ydesc(0, it).start()

                @pl.when(mx == 1)
                def _():
                    pl.semaphore_signal(xready, inc=1, device_id=xnbr,
                                        device_id_type=_MESH)
            else:
                if j in group_of_first_chunk:
                    loads[group_of_first_chunk[j]].wait()
                sbuf[pl.ds(soff(j), C), :] = out_ref[
                    rows(own, soff(j), C), :].astype(jnp.bfloat16)
                for it in items[j]:
                    ydesc(j, it).start()

        def xwait(row0, c0, f):
            piece = rbuf.at[pl.ds(row0, C), pl.ds(c0, W)]
            pltpu.make_async_remote_copy(
                src_ref=piece, dst_ref=piece, send_sem=fssem,
                recv_sem=frsem.at[f], device_id=xnbr,
                device_id_type=_MESH).wait_recv()

        def xproc(j):
            if j < nF:
                for p in range(NC):
                    xwait(foff(j), p * W, j * NC + p)
                row0 = foff(j)
            else:
                for p in range(nBp):
                    xwait(F, pl.multiple_of((1 - mx) * (n - Wf) + p * W, W),
                          nF * NC + p)
                row0 = F
            out_ref[rows(oth, row0, C), :] = rbuf[pl.ds(row0, C), :].astype(jnp.float32)

        nX = nF + 1
        sent = 0
        while sent < min(_N_PRIME, nS):
            send(sent)
            sent += 1
        xdone = 0
        for j in range(nS):
            if j == nS - 1:
                pltpu.make_async_copy(sbuf.at[pl.ds(0, S - C)],
                                      sbuf.at[pl.ds(0, S - C)], ssem).wait()
                for it in items[nF]:
                    ydesc(nF, it).wait_send()
                rest.wait()
            for k, it in enumerate(items[j]):
                ydesc(j, it).wait_recv()
                if it[2]:
                    if j == 0 and k == 0:
                        @pl.when(mx == 0)
                        def _():
                            pl.semaphore_wait(xready, 1)
                    fdesc(j, it).start()
            for _ in range(_SENDS_PER_STEP):
                if sent < nS:
                    send(sent)
                    sent += 1
            if j != nF:
                out_ref[rows(oth, soff(j), C), :] = rbuf[
                    pl.ds(soff(j), C), :].astype(jnp.float32)
            lag = nMid + (_X_MARGIN if j < nF else 0)
            while xdone <= j - lag and xdone < nX - 1:
                xproc(xdone)
                xdone += 1
        while xdone < nX - 1:
            xproc(xdone)
            xdone += 1
        pltpu.make_async_copy(rbuf.at[pl.ds(0, F)], rbuf.at[pl.ds(0, F)],
                              fssem).wait()
        for it in items[nF]:
            if it[2]:
                fdesc(nF, it).wait_send()
        xproc(nX - 1)

    n_recv = nF * NC + nBp + nBd + (nMid - 1)
    return pl.pallas_call(
        body,
        out_shape=jax.ShapeDtypeStruct((2 * m, n), x.dtype),
        in_specs=[pl.BlockSpec(memory_space=pl.ANY)],
        out_specs=pl.BlockSpec(memory_space=pltpu.VMEM),
        scratch_shapes=[
            pltpu.VMEM((m, n), jnp.bfloat16),
            pltpu.VMEM((m, n), jnp.bfloat16),
            pltpu.SemaphoreType.DMA((nG + 2,)),
            pltpu.SemaphoreType.DMA,
            pltpu.SemaphoreType.DMA((nBp + nBd,)),
            pltpu.SemaphoreType.DMA((n_recv,)),
            pltpu.SemaphoreType.DMA,
            pltpu.SemaphoreType.DMA((nBp,)),
            pltpu.SemaphoreType.DMA((nF * NC + nBp,)),
            pltpu.SemaphoreType.REGULAR,
        ],
        compiler_params=_compiler_params(),
    )(x)
```
